```python
import numpy as np

kernel_name = "dist_ar_i_i_m256_n256"

def setup_inputs():
    return {"x": np.random.randn(1024, 256).astype(np.float32)}

def reference(x: np.ndarray) -> np.ndarray:
    return x.reshape(4, 256, 256).sum(axis=0)
```

```python
import jax
import jax.numpy as jnp
from jax import lax
from jax.experimental import pallas as pl
from jax.experimental.pallas import tpu as pltpu

MESH = pl.DeviceIdType.MESH
M = N = 256
HC = 128
CR = 16
NCH = M // CR
LOADS = (16, 16, 32, 64, 128)


def pallas_dist_ar_i_i_m256_n256_kernel(x: jax.Array):
    def body(x_ref, o_ref, xv, s1, r1, s2, r2, lsem, ssem, r1sem, r2sem, hsem):
        me = lax.axis_index("i")
        yp = me ^ 1
        xp = 3 - me
        bs = pltpu.get_barrier_semaphore()

        lcps = []
        off = 0
        for i, n in enumerate(LOADS):
            cp = pltpu.make_async_copy(
                x_ref.at[pl.ds(off, n)], xv.at[pl.ds(off, n)], lsem.at[i]
            )
            lcps.append((off, n, cp))
            off += n

        def rows(c):
            return pl.ds(c * CR, CR)

        def cols(h):
            return pl.ds(h * HC, HC)

        def cp1(h, c):
            return pltpu.make_async_remote_copy(
                s1.at[h, c], r1.at[h, c], ssem.at[0], r1sem.at[h, c],
                device_id=(yp if h == 0 else xp,), device_id_type=MESH,
            )

        def cp2(h, c):
            return pltpu.make_async_remote_copy(
                s2.at[h, c], r2.at[h, c], ssem.at[1], r2sem.at[h, c],
                device_id=(xp if h == 0 else yp,), device_id_type=MESH,
            )

        def conv(h, c):
            s1[h, c] = xv[rows(c), cols(h)].astype(jnp.bfloat16)

        def mid(h, c):
            cp1(h, c).wait_recv()
            t = xv[rows(c), cols(h)] + r1[h, c].astype(jnp.float32)
            s2[h, c] = t.astype(jnp.bfloat16)
            cp2(h, c).start()
            xv[rows(c), cols(h)] = t

        def fin(h, c):
            cp2(h, c).wait_recv()
            o_ref[rows(c), cols(h)] = xv[rows(c), cols(h)] + r2[h, c].astype(
                jnp.float32
            )

        def sig(sem, dev):
            pl.semaphore_signal(sem, inc=1, device_id=(dev,), device_id_type=MESH)

        def role_ad(is_a):
            if is_a:
                sig(bs, yp)
                sig(bs, xp)
            for _, _, cp in lcps:
                cp.start()
            if is_a:
                for off, n, cp in lcps:
                    cp.wait()
                    for c in range(off // CR, (off + n) // CR):
                        conv(0, c)
                        conv(1, c)
                pl.semaphore_wait(bs, 2)
                for c in range(NCH):
                    cp1(0, c).start()
                    cp1(1, c).start()
            else:
                pl.semaphore_wait(bs, 2)
                sig(hsem, yp)
                sig(hsem, xp)
                for off, n, cp in lcps:
                    cp.wait()
                    for c in range(off // CR, (off + n) // CR):
                        conv(0, c)
                        cp1(0, c).start()
                        conv(1, c)
                        cp1(1, c).start()
            for c in range(NCH):
                mid(0, c)
                mid(1, c)
            for c in range(NCH):
                fin(0, c)
                fin(1, c)

        def role_bc(ha):
            hd = 1 - ha
            sig(bs, yp)
            sig(bs, xp)
            for _, _, cp in lcps:
                cp.start()
            pl.semaphore_wait(bs, 1)
            for off, n, cp in lcps:
                cp.wait()
                for c in range(off // CR, (off + n) // CR):
                    conv(ha, c)
                    cp1(ha, c).start()
            for c in range(NCH):
                conv(hd, c)
            pl.semaphore_wait(hsem, 1)
            for c in range(NCH):
                cp1(hd, c).start()
            for c in range(NCH):
                mid(hd, c)
                mid(ha, c)
            for c in range(NCH):
                fin(hd, c)
            for c in range(NCH):
                fin(ha, c)

        pl.when(me == 0)(lambda: role_ad(True))
        pl.when(me == 2)(lambda: role_ad(False))
        pl.when(me == 1)(lambda: role_bc(0))
        pl.when(me == 3)(lambda: role_bc(1))
        pltpu.make_async_copy(s1, s1, ssem.at[0]).wait()
        pltpu.make_async_copy(s2, s2, ssem.at[1]).wait()

    bshape = (2, NCH, CR, HC)
    return pl.pallas_call(
        body,
        out_shape=jax.ShapeDtypeStruct((M, N), jnp.float32),
        in_specs=[pl.BlockSpec(memory_space=pl.ANY)],
        out_specs=pl.BlockSpec(memory_space=pltpu.VMEM),
        scratch_shapes=[pltpu.VMEM((M, N), jnp.float32)]
        + [pltpu.VMEM(bshape, jnp.bfloat16)] * 4
        + [
            pltpu.SemaphoreType.DMA((len(LOADS),)),
            pltpu.SemaphoreType.DMA((2,)),
            pltpu.SemaphoreType.DMA((2, NCH)),
            pltpu.SemaphoreType.DMA((2, NCH)),
            pltpu.SemaphoreType.REGULAR,
        ],
        compiler_params=pltpu.CompilerParams(
            collective_id=0,
            disable_bounds_checks=True,
            disable_semaphore_checks=True,
        ),
    )(x)
```

```python
import functools

import jax
import jax.numpy as jnp
from jax import lax
from jax.experimental import pallas as pl
from jax.experimental.pallas import tpu as pltpu

MESH = pl.DeviceIdType.MESH
BF16 = jnp.bfloat16
F32 = jnp.float32

M = N = 256
HC = 128
T = 8
NT = M // T

DEV_A, DEV_C, DEV_D, DEV_B = 0, 1, 2, 3

LOADS = ((0, 8), (8, 8), (16, 16), (32, 32), (64, 64), (128, 128))
N_EARLY = 4

CR = 16
NC = M // CR
NC_F32 = 1
NC_BF = NC - NC_F32
COARSE_TO_A = tuple(range(NC_BF, NC)) + tuple(range(NC_BF))

SR = 2
F32_ROWS = 16
F0 = M - F32_ROWS
STREAM = tuple((r, True) for r in range(F0, M, SR)) + tuple(
    (r, False) for r in range(0, F0, SR)
)
NS = len(STREAM)
TILE_ORDER = tuple(range(F0 // T, NT)) + tuple(range(F0 // T))
SLOT = {t: q for q, t in enumerate(TILE_ORDER)}
GROUPS = (4, 4, 4, 4, 4, 4, 4, 2, 1, 1)
NG = len(GROUPS)
G0 = tuple(sum(GROUPS[:g]) for g in range(NG))
SLOT_GROUP = tuple(g for g in range(NG) for _ in range(GROUPS[g]))
LAG = 128

S1C, S2C, S1F, S2F, SF32 = 0, 2, 4, 6, 8


def _body(
    x_ref, o_ref, xv, s1c, r1c, s2c, r2c, s1f, r1f, s2f, r2f, rf, raf,
    lsem, ssem, r1csem, r2csem, r1fsem, r2fsem, hsem,
):
    def signal(sem, dev):
        pl.semaphore_signal(sem, inc=1, device_id=(dev,), device_id_type=MESH)

    barrier = pltpu.get_barrier_semaphore()
    signal(barrier, DEV_D)

    loads = [
        pltpu.make_async_copy(
            x_ref.at[pl.ds(r, n)], xv.at[pl.ds(r, n)], lsem.at[i]
        )
        for i, (r, n) in enumerate(LOADS)
    ]
    for cp in loads[:N_EARLY]:
        cp.start()

    def cols(h):
        return pl.ds(h * HC, HC)

    def crows(c):
        return pl.ds(c * CR, CR)

    def role(me):
        y_nbr, x_nbr = me ^ 1, 3 - me
        step1 = (y_nbr, x_nbr)
        step2 = (x_nbr, y_nbr)

        def remote(src, dst, si, rsem, dev):
            return pltpu.make_async_remote_copy(
                src, dst, ssem.at[si], rsem, device_id=(dev,), device_id_type=MESH
            )

        def copy1c(h, c):
            return remote(s1c.at[h, c], r1c.at[h, c], S1C + h, r1csem.at[h, c], step1[h])

        def copy1c_f32(h, c):
            return remote(
                x_ref.at[crows(c), cols(h)], raf.at[h, c - NC_BF],
                SF32 + h, r1csem.at[h, c], step1[h],
            )

        def copy2c(h, c):
            return remote(s2c.at[h, c], r2c.at[h, c], S2C + h, r2csem.at[h, c], step2[h])

        def copy1f(h, i):
            r, is_f32 = STREAM[i]
            if is_f32:
                return remote(
                    x_ref.at[pl.ds(r, SR), cols(h)], rf.at[pl.ds(r - F0, SR)],
                    SF32 + h, r1fsem.at[i], step1[h],
                )
            q, s = SLOT[r // T], pl.ds(r % T, SR)
            return remote(s1f.at[h, q, s], r1f.at[q, s], S1F + h, r1fsem.at[i], step1[h])

        def copy2f(h, i):
            r, _ = STREAM[i]
            q, s = SLOT[r // T], pl.ds(r % T, SR)
            return remote(
                s2f.at[q, s], r2f.at[h, q, s],
                S2F + h, r2fsem.at[h, SLOT_GROUP[q]], step2[h],
            )

        def wait_total(ref, sem):
            pltpu.make_async_copy(ref, ref, sem).wait()

        def pack_c(h, c):
            s1c[h, c] = xv[crows(c), cols(h)].astype(BF16)

        def forward_c(h, c):
            if me == DEV_A and c >= NC_BF:
                copy1c_f32(h, c).wait_recv()
                y = raf[h, c - NC_BF]
            else:
                copy1c(h, c).wait_recv()
                y = r1c[h, c].astype(F32)
            t = xv[crows(c), cols(h)] + y
            s2c[h, c] = t.astype(BF16)
            copy2c(h, c).start()
            xv[crows(c), cols(h)] = t

        def forward_f(h, i):
            r, is_f32 = STREAM[i]
            q, s = SLOT[r // T], pl.ds(r % T, SR)
            copy1f(h, i).wait_recv()
            y = rf[pl.ds(r - F0, SR), :] if is_f32 else r1f[q, s].astype(F32)
            t = xv[pl.ds(r, SR), cols(h)] + y
            s2f[q, s] = t.astype(BF16)
            copy2f(h, i).start()
            xv[pl.ds(r, SR), cols(h)] = t

        def finish_c(h, c):
            copy2c(h, c).wait_recv()
            o_ref[crows(c), cols(h)] = xv[crows(c), cols(h)] + r2c[h, c].astype(F32)

        def finish_f(h, g):
            wait_total(r2f.at[h, pl.ds(G0[g], GROUPS[g])], r2fsem.at[h, g])
            for q in range(G0[g], G0[g] + GROUPS[g]):
                rows = pl.ds(TILE_ORDER[q] * T, T)
                o_ref[rows, cols(h)] = xv[rows, cols(h)] + r2f[h, q].astype(F32)

        if me == DEV_A:
            signal(barrier, DEV_C)
            signal(barrier, DEV_B)
            for cp in loads[N_EARLY:]:
                cp.start()
            for cp in loads:
                cp.wait()
            for c in range(NC):
                pack_c(0, c)
                pack_c(1, c)
            pl.semaphore_wait(barrier, 2)
            for c in range(NC):
                copy1c(0, c).start()
                copy1c(1, c).start()
            for c in COARSE_TO_A:
                forward_c(0, c)
                forward_c(1, c)
            for h in (0, 1):
                wait_total(s1c.at[h], ssem.at[S1C + h])
            for g in range(NG):
                if g == NG - 3:
                    for h in (0, 1):
                        wait_total(s2c.at[h], ssem.at[S2C + h])
                finish_f(0, g)
                finish_f(1, g)

        elif me == DEV_D:
            pl.semaphore_wait(barrier, 4)
            for i in range(NS):
                if STREAM[i][1]:
                    copy1f(0, i).start()
                    copy1f(1, i).start()
            signal(hsem, DEV_B)
            signal(hsem, DEV_C)
            for cp in loads[N_EARLY:]:
                cp.start()
            for (r0, n), cp in zip(LOADS, loads):
                cp.wait()
                for t in range(r0 // T, min(r0 + n, F0) // T):
                    idx = [i for i in range(NS) if STREAM[i][0] // T == t]
                    for h in (0, 1):
                        s1f[h, SLOT[t]] = xv[pl.ds(t * T, T), cols(h)].astype(BF16)
                        if t == 0:
                            copy1f(h, idx[0]).start()
                    for i in idx[1:] if t == 0 else idx:
                        copy1f(0, i).start()
                        copy1f(1, i).start()
            for c in range(NC):
                forward_c(0, c)
                forward_c(1, c)
            for c in range(NC):
                finish_c(0, c)
                finish_c(1, c)
            for h in (0, 1):
                wait_total(rf, ssem.at[SF32 + h])
                wait_total(
                    s1f.at[h, pl.ds(F32_ROWS // T, F0 // T)], ssem.at[S1F + h]
                )
                wait_total(s2c.at[h], ssem.at[S2C + h])

        else:
            ha = step1.index(DEV_A)
            hd = 1 - ha
            signal(barrier, DEV_A)
            pl.semaphore_wait(barrier, 1)
            for c in range(NC_BF, NC):
                copy1c_f32(ha, c).start()
            for cp in loads[N_EARLY:]:
                cp.start()
            for (r0, n), cp in zip(LOADS, loads):
                cp.wait()
                for c in range(NC_BF):
                    if r0 < (c + 1) * CR <= r0 + n:
                        pack_c(ha, c)
                        copy1c(ha, c).start()
            for c in range(NC):
                pack_c(hd, c)
            pl.semaphore_wait(hsem, 1)
            for c in range(NC):
                copy1c(hd, c).start()
            nxt = 0
            for i in range(NS):
                forward_f(hd, i)
                if nxt < NC and (i + 1) * SR >= LAG + nxt * CR:
                    forward_c(ha, nxt)
                    nxt += 1
            for c in range(nxt, NC):
                forward_c(ha, c)
            for c in COARSE_TO_A:
                finish_c(hd, c)
            for c in range(NC):
                finish_c(ha, c)
            wait_total(raf.at[ha], ssem.at[SF32 + ha])
            wait_total(s1c.at[ha, pl.ds(0, NC_BF)], ssem.at[S1C + ha])
            wait_total(s1c.at[hd], ssem.at[S1C + hd])
            wait_total(s2c.at[ha], ssem.at[S2C + ha])
            wait_total(s2f, ssem.at[S2F + hd])

    me = lax.axis_index("i")
    for dev in (DEV_C, DEV_B, DEV_D, DEV_A):
        pl.when(me == dev)(functools.partial(role, dev))


def pallas_dist_ar_i_i_m256_n256_kernel(x: jax.Array):
    dma = pltpu.SemaphoreType.DMA
    coarse = pltpu.VMEM((2, NC, CR, HC), BF16)
    return pl.pallas_call(
        _body,
        out_shape=jax.ShapeDtypeStruct((M, N), F32),
        in_specs=[pl.BlockSpec(memory_space=pl.ANY)],
        out_specs=pl.BlockSpec(memory_space=pltpu.VMEM),
        scratch_shapes=[
            pltpu.VMEM((M, N), F32),
            coarse,
            coarse,
            coarse,
            coarse,
            pltpu.VMEM((2, NT, T, HC), BF16),
            pltpu.VMEM((NT, T, HC), BF16),
            pltpu.VMEM((NT, T, HC), BF16),
            pltpu.VMEM((2, NT, T, HC), BF16),
            pltpu.VMEM((F32_ROWS, HC), F32),
            pltpu.VMEM((2, NC_F32, CR, HC), F32),
            dma((len(LOADS),)),
            dma((10,)),
            dma((2, NC)),
            dma((2, NC)),
            dma((NS,)),
            dma((2, NG)),
            pltpu.SemaphoreType.REGULAR,
        ],
        compiler_params=pltpu.CompilerParams(
            collective_id=0,
            disable_bounds_checks=True,
            disable_semaphore_checks=True,
        ),
    )(x)
```

```python
import functools

import jax
import jax.numpy as jnp
from jax import lax
from jax.experimental import pallas as pl
from jax.experimental.pallas import tpu as pltpu

MESH = pl.DeviceIdType.MESH
BF16 = jnp.bfloat16
F32 = jnp.float32

M = N = 256
HC = 128
T = 8
NT = M // T

DEV_A, DEV_C, DEV_D, DEV_B = 0, 1, 2, 3

LOADS = ((0, 8), (8, 8), (16, 16), (32, 32), (64, 64), (128, 128))
N_FIRST = 4
LOADS_D = ((0, 32), (32, 32), (64, 64), (128, 128))

CR = 16
NC = M // CR
NC_F32 = 1
NC_BF = NC - NC_F32
COARSE_TO_A = tuple(range(NC_BF, NC)) + tuple(range(NC_BF))

SR = 2
SUB = T // SR
NF32 = 2
HEAD = ((23, 30, 5, 9, 3, 12, 16, 27), (23, 28, 5, 9, 14, 18, 19, 2))
NE = len(HEAD[0]) - NF32
TILES = tuple(hd + tuple(t for t in range(NT) if t not in hd) for hd in HEAD)
GROUPS = (4, 4, 4, 4, 4, 4, 4, 2, 1, 1)
NG = len(GROUPS)
G0 = tuple(sum(GROUPS[:g]) for g in range(NG))
GROUP_OF = tuple(g for g in range(NG) for _ in range(GROUPS[g]))
LAG = 128

S1C, S2C, S1F, S2F, SF32 = 0, 2, 4, 6, 8


def _body(
    x_ref, o_ref, xv, xe, s1c, r1c, s2c, r2c, s1f, r1f, s2f, r2f, rf, raf,
    lsem, esem, ssem, r1csem, r2csem, r1fsem, r2fsem, hsem,
):
    def signal(sem, dev):
        pl.semaphore_signal(sem, inc=1, device_id=(dev,), device_id_type=MESH)

    def cols(h):
        return pl.ds(h * HC, HC)

    def crows(c):
        return pl.ds(c * CR, CR)

    def trows(h, q):
        return pl.ds(TILES[h][q] * T, T)

    def prows(h, q, j):
        return pl.ds(TILES[h][q] * T + j * SR, SR)

    def piece(j):
        return pl.ds(j * SR, SR)

    def make_loads(spec):
        return [
            pltpu.make_async_copy(
                x_ref.at[pl.ds(r, n)], xv.at[pl.ds(r, n)], lsem.at[i]
            )
            for i, (r, n) in enumerate(spec)
        ]

    def early_loads(e):
        q = NF32 + e
        if TILES[0][q] == TILES[1][q]:
            return [pltpu.make_async_copy(x_ref.at[trows(0, q)], xe.at[e], esem.at[0, e])]
        return [
            pltpu.make_async_copy(
                x_ref.at[trows(h, q), cols(h)], xe.at[e, :, cols(h)], esem.at[h, e]
            )
            for h in (0, 1)
        ]

    barrier = pltpu.get_barrier_semaphore()
    signal(barrier, DEV_D)
    for cp in early_loads(0):
        cp.start()

    def role(me):
        y_nbr, x_nbr = me ^ 1, 3 - me
        step1 = (y_nbr, x_nbr)
        step2 = (x_nbr, y_nbr)

        def remote(src, dst, si, rsem, dev):
            return pltpu.make_async_remote_copy(
                src, dst, ssem.at[si], rsem, device_id=(dev,), device_id_type=MESH
            )

        def copy1c(h, c):
            return remote(s1c.at[h, c], r1c.at[h, c], S1C + h, r1csem.at[h, c], step1[h])

        def copy1c_f32(h, c):
            return remote(
                x_ref.at[crows(c), cols(h)], raf.at[h, c - NC_BF],
                SF32 + h, r1csem.at[h, c], step1[h],
            )

        def copy2c(h, c):
            return remote(s2c.at[h, c], r2c.at[h, c], S2C + h, r2csem.at[h, c], step2[h])

        def copy1f(h, q, j):
            rsem = r1fsem.at[q * SUB + j]
            if q < NF32:
                return remote(
                    x_ref.at[prows(h, q, j), cols(h)], rf.at[q, piece(j)],
                    SF32 + h, rsem, step1[h],
                )
            return remote(
                s1f.at[h, q, piece(j)], r1f.at[q, piece(j)], S1F + h, rsem, step1[h]
            )

        def copy2f(h, q, j):
            return remote(
                s2f.at[q, piece(j)], r2f.at[h, q, piece(j)],
                S2F + h, r2fsem.at[h, GROUP_OF[q]], step2[h],
            )

        def wait_total(ref, sem):
            pltpu.make_async_copy(ref, ref, sem).wait()

        def pack_c(h, c):
            s1c[h, c] = xv[crows(c), cols(h)].astype(BF16)

        def forward_c(h, c):
            if me == DEV_A and c >= NC_BF:
                copy1c_f32(h, c).wait_recv()
                y = raf[h, c - NC_BF]
            else:
                copy1c(h, c).wait_recv()
                y = r1c[h, c].astype(F32)
            t = xv[crows(c), cols(h)] + y
            s2c[h, c] = t.astype(BF16)
            copy2c(h, c).start()
            xv[crows(c), cols(h)] = t

        def forward_f(h, q, j):
            copy1f(h, q, j).wait_recv()
            y = rf[q, piece(j)] if q < NF32 else r1f[q, piece(j)].astype(F32)
            t = xv[prows(h, q, j), cols(h)] + y
            s2f[q, piece(j)] = t.astype(BF16)
            copy2f(h, q, j).start()
            xv[prows(h, q, j), cols(h)] = t

        def finish_c(h, c):
            copy2c(h, c).wait_recv()
            o_ref[crows(c), cols(h)] = xv[crows(c), cols(h)] + r2c[h, c].astype(F32)

        def finish_f(h, g):
            wait_total(r2f.at[h, pl.ds(G0[g], GROUPS[g])], r2fsem.at[h, g])
            for q in range(G0[g], G0[g] + GROUPS[g]):
                rows = trows(h, q)
                o_ref[rows, cols(h)] = xv[rows, cols(h)] + r2f[h, q].astype(F32)

        if me == DEV_A:
            signal(barrier, DEV_C)
            signal(barrier, DEV_B)
            loads = make_loads(LOADS)
            for cp in loads:
                cp.start()
            for cp in early_loads(0) + loads:
                cp.wait()
            for c in range(NC):
                pack_c(0, c)
                pack_c(1, c)
            pl.semaphore_wait(barrier, 2)
            for c in range(NC):
                copy1c(0, c).start()
                copy1c(1, c).start()
            for c in COARSE_TO_A:
                forward_c(0, c)
                forward_c(1, c)
            for h in (0, 1):
                wait_total(s1c.at[h], ssem.at[S1C + h])
            for g in range(NG):
                if g == NG - 3:
                    for h in (0, 1):
                        wait_total(s2c.at[h], ssem.at[S2C + h])
                finish_f(0, g)
                finish_f(1, g)

        elif me == DEV_D:
            for e in range(1, NE):
                for cp in early_loads(e):
                    cp.start()
            pl.semaphore_wait(barrier, 4)
            for q in range(NF32):
                for j in range(SUB):
                    copy1f(0, q, j).start()
                    copy1f(1, q, j).start()
            signal(hsem, DEV_B)
            signal(hsem, DEV_C)
            loads = make_loads(LOADS_D)
            for cp in loads:
                cp.start()
            for e in range(NE):
                q = NF32 + e
                for cp in early_loads(e):
                    cp.wait()
                for h in (0, 1):
                    s1f[h, q] = xe[e, :, cols(h)].astype(BF16)
                    copy1f(h, q, 0).start()
                for j in range(1, SUB):
                    copy1f(0, q, j).start()
                    copy1f(1, q, j).start()
            nxt = [NF32 + NE, NF32 + NE]
            for (r0, n), cp in zip(LOADS_D, loads):
                cp.wait()
                ready = [
                    [q for q in range(nxt[h], NT) if (TILES[h][q] + 1) * T <= r0 + n]
                    for h in (0, 1)
                ]
                for k in range(max(len(ready[0]), len(ready[1]))):
                    for h in (0, 1):
                        if k < len(ready[h]):
                            q = ready[h][k]
                            s1f[h, q] = xv[trows(h, q), cols(h)].astype(BF16)
                            for j in range(SUB):
                                copy1f(h, q, j).start()
                nxt = [nxt[h] + len(ready[h]) for h in (0, 1)]
            for c in range(NC):
                forward_c(0, c)
                forward_c(1, c)
            for c in range(NC):
                finish_c(0, c)
                finish_c(1, c)
            for h in (0, 1):
                wait_total(rf, ssem.at[SF32 + h])
                wait_total(s1f.at[h, pl.ds(NF32, NT - NF32)], ssem.at[S1F + h])
                wait_total(s2c.at[h], ssem.at[S2C + h])

        else:
            ha = step1.index(DEV_A)
            hd = 1 - ha
            signal(barrier, DEV_A)
            loads = make_loads(LOADS)
            for cp in loads[:N_FIRST]:
                cp.start()
            pl.semaphore_wait(barrier, 1)
            for c in range(NC_BF, NC):
                copy1c_f32(ha, c).start()
            for cp in loads[N_FIRST:]:
                cp.start()
            for (r0, n), cp in zip(LOADS, loads):
                cp.wait()
                for c in range(NC_BF):
                    if r0 < (c + 1) * CR <= r0 + n:
                        pack_c(ha, c)
                        copy1c(ha, c).start()
            for cp in early_loads(0):
                cp.wait()
            for c in range(NC):
                pack_c(hd, c)
            pl.semaphore_wait(hsem, 1)
            for c in range(NC):
                copy1c(hd, c).start()
            nxt = 0
            for q in range(NT):
                for j in range(SUB):
                    forward_f(hd, q, j)
                if nxt < NC and (q + 1) * T >= LAG + nxt * CR:
                    forward_c(ha, nxt)
                    nxt += 1
            for c in range(nxt, NC):
                forward_c(ha, c)
            for c in COARSE_TO_A:
                finish_c(hd, c)
            for c in range(NC):
                finish_c(ha, c)
            wait_total(raf.at[ha], ssem.at[SF32 + ha])
            wait_total(s1c.at[ha, pl.ds(0, NC_BF)], ssem.at[S1C + ha])
            wait_total(s1c.at[hd], ssem.at[S1C + hd])
            wait_total(s2c.at[ha], ssem.at[S2C + ha])
            wait_total(s2f, ssem.at[S2F + hd])

    me = lax.axis_index("i")
    for dev in (DEV_D, DEV_C, DEV_B, DEV_A):
        pl.when(me == dev)(functools.partial(role, dev))


def pallas_dist_ar_i_i_m256_n256_kernel(x: jax.Array):
    dma = pltpu.SemaphoreType.DMA
    coarse = pltpu.VMEM((2, NC, CR, HC), BF16)
    return pl.pallas_call(
        _body,
        out_shape=jax.ShapeDtypeStruct((M, N), F32),
        in_specs=[pl.BlockSpec(memory_space=pl.ANY)],
        out_specs=pl.BlockSpec(memory_space=pltpu.VMEM),
        scratch_shapes=[
            pltpu.VMEM((M, N), F32),
            pltpu.VMEM((NE, T, N), F32),
            coarse,
            coarse,
            coarse,
            coarse,
            pltpu.VMEM((2, NT, T, HC), BF16),
            pltpu.VMEM((NT, T, HC), BF16),
            pltpu.VMEM((NT, T, HC), BF16),
            pltpu.VMEM((2, NT, T, HC), BF16),
            pltpu.VMEM((NF32, T, HC), F32),
            pltpu.VMEM((2, NC_F32, CR, HC), F32),
            dma((len(LOADS),)),
            dma((2, NE)),
            dma((10,)),
            dma((2, NC)),
            dma((2, NC)),
            dma((NT * SUB,)),
            dma((2, NG)),
            pltpu.SemaphoreType.REGULAR,
        ],
        compiler_params=pltpu.CompilerParams(
            collective_id=0,
            disable_bounds_checks=True,
            disable_semaphore_checks=True,
        ),
    )(x)
```

```python
import functools

import jax
import jax.numpy as jnp
from jax import lax
from jax.experimental import pallas as pl
from jax.experimental.pallas import tpu as pltpu

MESH = pl.DeviceIdType.MESH
BF16 = jnp.bfloat16
F32 = jnp.float32

M = N = 256
HC = 128
T = 8
NT = M // T

DEV_A, DEV_C, DEV_D, DEV_B = 0, 1, 2, 3

LOADS = ((0, 32), (32, 32), (64, 64), (128, 128))

HEAD = ((23, 30, 5, 9, 3, 12, 16, 27), (23, 28, 5, 9, 14, 18, 19, 2))


def _order(first):
    return tuple(first) + tuple(t for t in range(NT) if t not in first)


NF32 = 2
NE = len(HEAD[0]) - NF32
TILES = tuple(_order(hd) for hd in HEAD)
SR = 2
SUB = T // SR
DIRECT = (
    ((31, 1, 1), (31, 2, 2)),
    ((9, 0, 4), (10, 0, 2), (20, 0, 4), (21, 0, 2), (31, 1, 1), (31, 2, 2)),
)
ND = max(len(d) for d in DIRECT)
IS_DIRECT = tuple(
    frozenset((q, j) for q, j0, n in d for j in range(j0, j0 + n)) for d in DIRECT
)
GROUPS = (4, 4, 4, 4, 4, 4, 4, 2, 1, 1)
NG = len(GROUPS)
G0 = tuple(sum(GROUPS[:g]) for g in range(NG))
GROUP_OF = tuple(g for g in range(NG) for _ in range(GROUPS[g]))

NAF = 3
NAE = 5
ATILES = tuple(_order(hd[:NF32] + hd[NF32 + NAE :] + hd[NF32 : NF32 + NAE]) for hd in HEAD)

CR = 16
NC = M // CR
TPC = CR // T
CORDER = tuple(
    tuple(
        sorted(
            range(NC),
            key=lambda c, at=at: max(at.index(t) for t in range(c * TPC, (c + 1) * TPC)),
        )
    )
    for at in ATILES
)
LAG = 128

S1C, S2C, S1F, S2F, S1A = 0, 2, 4, 6, 7
SF32 = 8
SDIR = SF32 + 2 * NF32 * SUB
N_SSEM = SDIR + 2 * ND
assert NAF <= 2 * NF32 * SUB and NF32 + NAE + NAF - NF32 == len(HEAD[0])
assert TILES[0][NF32] == TILES[1][NF32]


def _body(
    x_ref, o_ref, xv, xe, s1c, r1c, s2c, r2c, s1f, r1f, s2f, r2f, s1a, r1a,
    rf, raf, rx,
    lsem, esem, ssem, r1csem, r2csem, r1fsem, r2fsem, rasem, rxsem, hsem,
):
    def signal(sem, dev):
        pl.semaphore_signal(sem, inc=1, device_id=(dev,), device_id_type=MESH)

    def cols(h):
        return pl.ds(h * HC, HC)

    def crows(c):
        return pl.ds(c * CR, CR)

    def tile(t):
        return pl.ds(t * T, T)

    def prows(h, q, j, n=1):
        return pl.ds(TILES[h][q] * T + j * SR, n * SR)

    def piece(j, n=1):
        return pl.ds(j * SR, n * SR)

    def early_load(e, h=None):
        if h is None:
            rows = tile(TILES[0][NF32 + e])
            return pltpu.make_async_copy(x_ref.at[rows], xe.at[e], esem.at[0, e])
        return pltpu.make_async_copy(
            x_ref.at[tile(TILES[h][NF32 + e]), cols(h)],
            xe.at[e, :, cols(h)],
            esem.at[h, e],
        )

    barrier = pltpu.get_barrier_semaphore()
    signal(barrier, DEV_D)
    early_load(0).start()

    def role(me):
        y_nbr, x_nbr = me ^ 1, 3 - me
        step1 = (y_nbr, x_nbr)
        step2 = (x_nbr, y_nbr)

        loads = [
            pltpu.make_async_copy(x_ref.at[pl.ds(r, n)], xv.at[pl.ds(r, n)], lsem.at[i])
            for i, (r, n) in enumerate(LOADS)
        ]

        def remote(src, dst, si, rsem, dev):
            return pltpu.make_async_remote_copy(
                src, dst, ssem.at[si], rsem, device_id=(dev,), device_id_type=MESH
            )

        def copy1c(h, c):
            return remote(s1c.at[h, c], r1c.at[h, c], S1C + h, r1csem.at[h, c], step1[h])

        def copy2c(h, c):
            return remote(s2c.at[h, c], r2c.at[h, c], S2C + h, r2csem.at[h, c], step2[h])

        def copy1a(h, p):
            if p < NAF:
                return remote(
                    x_ref.at[tile(ATILES[h][p]), cols(h)], raf.at[h, p],
                    SF32 + p, rasem.at[h, p], DEV_A,
                )
            return remote(s1a.at[p], r1a.at[h, p], S1A, rasem.at[h, p], DEV_A)

        def copy1f(h, q, j):
            rsem = r1fsem.at[q * SUB + j]
            if q < NF32:
                return remote(
                    x_ref.at[prows(h, q, j), cols(h)], rf.at[q, piece(j)],
                    SF32 + (h * NF32 + q) * SUB + j, rsem, step1[h],
                )
            return remote(
                s1f.at[h, q, piece(j)], r1f.at[q, piece(j)], S1F + h, rsem, step1[h]
            )

        def copy2f(h, q, j):
            return remote(
                s2f.at[q, piece(j)], r2f.at[h, q, piece(j)],
                S2F, r2fsem.at[h, GROUP_OF[q]], DEV_A,
            )

        def copy_direct(h, k):
            q, j, n = DIRECT[h][k]
            return remote(
                s1f.at[h, q, piece(j, n)], r2f.at[h, q, piece(j, n)],
                SDIR + h * ND + k, r2fsem.at[h, GROUP_OF[q]], DEV_A,
            )

        def copy_share(h, k):
            q, j, n = DIRECT[h][k]
            return remote(
                s2f.at[q, piece(j, n)], rx.at[h, k, piece(j, n)],
                S2F, rxsem.at[h, k], DEV_A,
            )

        def wait_total(ref, sem):
            pltpu.make_async_copy(ref, ref, sem).wait()

        def pack_c(h, c):
            s1c[h, c] = xv[crows(c), cols(h)].astype(BF16)

        def forward_c(h, c):
            copy1c(h, c).wait_recv()
            t = xv[crows(c), cols(h)] + r1c[h, c].astype(F32)
            s2c[h, c] = t.astype(BF16)
            copy2c(h, c).start()
            xv[crows(c), cols(h)] = t

        def forward_a(h, c):
            for k in range(TPC):
                p = ATILES[h].index(c * TPC + k)
                rows = tile(c * TPC + k)
                copy1a(h, p).wait_recv()
                y = raf[h, p] if p < NAF else r1a[h, p].astype(F32)
                t = xv[rows, cols(h)] + y
                s2c[h, c, tile(k)] = t.astype(BF16)
                xv[rows, cols(h)] = t
            copy2c(h, c).start()

        def forward_f(h, q, j):
            copy1f(h, q, j).wait_recv()
            y = rf[q, piece(j)] if q < NF32 else r1f[q, piece(j)].astype(F32)
            t = xv[prows(h, q, j), cols(h)] + y
            if (q, j) not in IS_DIRECT[h]:
                s2f[q, piece(j)] = t.astype(BF16)
                copy2f(h, q, j).start()
            xv[prows(h, q, j), cols(h)] = t

        def finish_c(h, c):
            copy2c(h, c).wait_recv()
            o_ref[crows(c), cols(h)] = xv[crows(c), cols(h)] + r2c[h, c].astype(F32)

        def finish_f(h, g):
            wait_total(r2f.at[h, pl.ds(G0[g], GROUPS[g])], r2fsem.at[h, g])
            for q in range(G0[g], G0[g] + GROUPS[g]):
                rows = tile(TILES[h][q])
                o_ref[rows, cols(h)] = xv[rows, cols(h)] + r2f[h, q].astype(F32)

        if me == DEV_A:
            signal(barrier, DEV_C)
            signal(barrier, DEV_B)
            for cp in loads:
                cp.start()
            early_load(0).wait()
            for cp in loads:
                cp.wait()
            for c in range(NC):
                pack_c(0, c)
                pack_c(1, c)
            pl.semaphore_wait(barrier, 2)
            for c in range(NC):
                copy1c(0, c).start()
                copy1c(1, c).start()
            for c0, c1 in zip(*CORDER):
                forward_a(0, c0)
                forward_a(1, c1)
            for h in (0, 1):
                for k, (q, j, n) in enumerate(DIRECT[h]):
                    copy_share(h, k).wait_recv()
                    rows = prows(h, q, j, n)
                    xv[rows, cols(h)] = xv[rows, cols(h)] + rx[h, k, piece(j, n)].astype(F32)
                wait_total(s1c.at[h], ssem.at[S1C + h])
            for g in range(NG):
                if g == NG - 3:
                    for h in (0, 1):
                        wait_total(s2c.at[h], ssem.at[S2C + h])
                finish_f(0, g)
                finish_f(1, g)

        elif me == DEV_D:

            def early(e):
                if TILES[0][NF32 + e] == TILES[1][NF32 + e]:
                    return [early_load(e)]
                return [early_load(e, 0), early_load(e, 1)]

            def send(h, q, j):
                if (q, j) not in IS_DIRECT[h]:
                    copy1f(h, q, j).start()
                elif h == 1:
                    for k, (qk, jk, _) in enumerate(DIRECT[h]):
                        if (qk, jk) == (q, j):
                            copy_direct(h, k).start()

            for e in range(1, NE):
                for cp in early(e):
                    cp.start()
            pl.semaphore_wait(barrier, 4)
            for q in range(NF32):
                for j in range(SUB):
                    copy1f(0, q, j).start()
                    copy1f(1, q, j).start()
            signal(hsem, DEV_B)
            signal(hsem, DEV_C)
            for cp in loads:
                cp.start()
            for e in range(NE):
                q = NF32 + e
                for cp in early(e):
                    cp.wait()
                for h in (0, 1):
                    s1f[h, q] = xe[e, :, cols(h)].astype(BF16)
                    send(h, q, 0)
                for j in range(1, SUB):
                    send(0, q, j)
                    send(1, q, j)
            for (r0, n), cp in zip(LOADS, loads):
                cp.wait()
                ready = [
                    [q for q in range(NF32 + NE, NT) if r0 <= TILES[h][q] * T < r0 + n]
                    for h in (0, 1)
                ]
                for i in range(max(len(ready[0]), len(ready[1]))):
                    for h in (0, 1):
                        if i < len(ready[h]):
                            q = ready[h][i]
                            s1f[h, q] = xv[tile(TILES[h][q]), cols(h)].astype(BF16)
                            for j in range(SUB):
                                send(h, q, j)
            for k in range(len(DIRECT[0])):
                copy_direct(0, k).start()
            for h in (0, 1):
                for q, j in sorted(IS_DIRECT[h]):
                    copy1f(h, q, j).start()
            for c in range(NC):
                forward_c(0, c)
                forward_c(1, c)
            for c in range(NC):
                finish_c(0, c)
                finish_c(1, c)
            for h in (0, 1):
                for q in range(NF32):
                    for j in range(SUB):
                        copy1f(h, q, j).wait_send()
                for k in range(len(DIRECT[h])):
                    copy_direct(h, k).wait_send()
                wait_total(s1f.at[h, pl.ds(NF32, NT - NF32)], ssem.at[S1F + h])
                wait_total(s2c.at[h], ssem.at[S2C + h])

        else:
            ha = step1.index(DEV_A)
            hd = 1 - ha
            for e in range(1, NAE):
                early_load(e, ha).start()
            pl.semaphore_wait(barrier, 1)
            for p in range(NAF):
                copy1a(ha, p).start()
            signal(barrier, DEV_A)
            for cp in loads:
                cp.start()
            for e in range(NAE):
                early_load(e, ha if e else None).wait()
                s1a[NAF + e] = xe[e, :, cols(ha)].astype(BF16)
                copy1a(ha, NAF + e).start()
            for (r0, n), cp in zip(LOADS, loads):
                cp.wait()
                for p in range(NAF + NAE, NT):
                    if r0 <= ATILES[ha][p] * T < r0 + n:
                        s1a[p] = xv[tile(ATILES[ha][p]), cols(ha)].astype(BF16)
                        copy1a(ha, p).start()
            for k, (q, j, n) in enumerate(DIRECT[hd]):
                s2f[q, piece(j, n)] = xv[prows(hd, q, j, n), cols(hd)].astype(BF16)
                copy_share(hd, k).start()
            for c in range(NC):
                pack_c(hd, c)
            pl.semaphore_wait(hsem, 1)
            for c in range(NC):
                copy1c(hd, c).start()
            nxt = 0
            for q in range(NT):
                for j in range(SUB):
                    if (q, j) not in IS_DIRECT[hd]:
                        forward_f(hd, q, j)
                if q < NT - 1 and (q + 1) * T >= LAG + nxt * CR:
                    forward_c(ha, nxt)
                    nxt += 1
            for c in range(nxt, NC):
                forward_c(ha, c)
            for q, j in sorted(IS_DIRECT[hd]):
                forward_f(hd, q, j)
            for c in CORDER[hd]:
                finish_c(hd, c)
            for c in range(NC):
                finish_c(ha, c)
            for p in range(NAF):
                copy1a(ha, p).wait_send()
            wait_total(s1a.at[pl.ds(NAF, NT - NAF)], ssem.at[S1A])
            wait_total(s1c.at[hd], ssem.at[S1C + hd])
            wait_total(s2c.at[ha], ssem.at[S2C + ha])
            wait_total(s2f, ssem.at[S2F])

    me = lax.axis_index("i")
    for dev in (DEV_D, DEV_C, DEV_B, DEV_A):
        pl.when(me == dev)(functools.partial(role, dev))


def pallas_dist_ar_i_i_m256_n256_kernel(x: jax.Array):
    dma = pltpu.SemaphoreType.DMA
    coarse = pltpu.VMEM((2, NC, CR, HC), BF16)
    one_half = pltpu.VMEM((NT, T, HC), BF16)
    two_halves = pltpu.VMEM((2, NT, T, HC), BF16)
    return pl.pallas_call(
        _body,
        out_shape=jax.ShapeDtypeStruct((M, N), F32),
        in_specs=[pl.BlockSpec(memory_space=pl.ANY)],
        out_specs=pl.BlockSpec(memory_space=pltpu.VMEM),
        scratch_shapes=[
            pltpu.VMEM((M, N), F32),
            pltpu.VMEM((NE, T, N), F32),
            coarse,
            coarse,
            coarse,
            coarse,
            two_halves,
            one_half,
            one_half,
            two_halves,
            one_half,
            two_halves,
            pltpu.VMEM((NF32, T, HC), F32),
            pltpu.VMEM((2, NAF, T, HC), F32),
            pltpu.VMEM((2, ND, T, HC), BF16),
            dma((len(LOADS),)),
            dma((2, NE)),
            dma((N_SSEM,)),
            dma((2, NC)),
            dma((2, NC)),
            dma((NT * SUB,)),
            dma((2, NG)),
            dma((2, NT)),
            dma((2, ND)),
            pltpu.SemaphoreType.REGULAR,
        ],
        compiler_params=pltpu.CompilerParams(
            collective_id=0,
            disable_bounds_checks=True,
            disable_semaphore_checks=True,
        ),
    )(x)
```
